```python
import numpy as np

kernel_name = "dist_max_ax1_xy_m4096_n1024"

def setup_inputs():
    return {"x": np.random.randn(8192, 2048).astype(np.float32)}

def reference(x: np.ndarray) -> np.ndarray:
    return np.max(x, axis=1, keepdims=True)
```

```python
import jax
import jax.numpy as jnp
from jax import lax
from jax.experimental import pallas as pl
from jax.experimental.pallas import tpu as pltpu

LANES = 128
SUBLANES = 8


def pallas_dist_max_ax1_xy_m4096_n1024_kernel(
x: jax.Array,
):
    m, n = x.shape
    half = m // 2
    raw = 128
    chunks1 = (1024, half - raw - 1024)
    chunks2 = (1024, 512, 256, 128)
    tail = (64, 32, 32)
    fin_after = (2, 3)
    raw_after = 1
    ncb = n // LANES

    chunks = chunks1 + chunks2 + tail
    n1 = len(chunks1)
    n2 = n1 + len(chunks2)
    nch = len(chunks)
    offs = [raw + sum(chunks[:i]) for i in range(nch)]
    assert offs[-1] + chunks[-1] == m and offs[n1] == half
    groups = []
    prev = 0
    for f in fin_after:
        end = sum(chunks2[:f + 1])
        groups.append((prev, end - prev))
        prev = end
    for b in range(sum(tail) // LANES):
        groups.append((prev + b * LANES, LANES))
    ng = len(groups)

    def body(x_hbm, out_ref, xbuf, rawbuf, part, rbuf,
             in_sems, p_send, p_recv, f_send, f_recv, r_send, r_recv):
        my_x = lax.axis_index("x")
        my_y = lax.axis_index("y")
        nbr = (my_x, 1 - my_y)
        base1 = pl.multiple_of(my_y * half, half)
        base2 = pl.multiple_of((1 - my_y) * half, half)

        def in_copy(c):
            g = (base1 + offs[c]) if c < n1 else (base2 + (offs[c] - half))
            return pltpu.make_async_copy(
                x_hbm.at[pl.ds(g, chunks[c]), :],
                xbuf.at[pl.ds(offs[c], chunks[c]), :],
                in_sems.at[c])

        for c in range(nch):
            in_copy(c).start()

        barrier = pltpu.get_barrier_semaphore()
        pl.semaphore_signal(barrier, inc=1, device_id=nbr,
                            device_id_type=pl.DeviceIdType.MESH)
        pl.semaphore_wait(barrier, 1)

        raw_rdma = pltpu.make_async_remote_copy(
            src_ref=x_hbm.at[pl.ds(base1, raw), :], dst_ref=rawbuf,
            send_sem=r_send, recv_sem=r_recv,
            device_id=nbr, device_id_type=pl.DeviceIdType.MESH)
        raw_rdma.start()

        part_rdma = pltpu.make_async_remote_copy(
            src_ref=part.at[:, pl.ds(raw, half - raw)],
            dst_ref=rbuf.at[:, pl.ds(raw, half - raw)],
            send_sem=p_send, recv_sem=p_recv,
            device_id=nbr, device_id_type=pl.DeviceIdType.MESH)

        def fin_rdma(g, base):
            s, l = groups[g]
            sl = out_ref.at[:, pl.ds(base + s, l)]
            return pltpu.make_async_remote_copy(
                src_ref=sl, dst_ref=sl,
                send_sem=f_send.at[g], recv_sem=f_recv.at[g],
                device_id=nbr, device_id_type=pl.DeviceIdType.MESH)

        def colmax(buf, r0, nr):
            vs = [buf[pl.ds(r0, nr), pl.ds(j * LANES, LANES)] for j in range(ncb)]
            while len(vs) > 1:
                vs = [jnp.maximum(vs[i], vs[i + 1]) for i in range(0, len(vs), 2)]
            return vs[0]

        def to_lanes(mat):
            return jnp.max(mat.T, axis=0, keepdims=True)

        def store_final(q, val):
            out_ref[:, pl.ds(pl.multiple_of(base2 + q, LANES), LANES)] = val

        diag = (lax.broadcasted_iota(jnp.int32, (SUBLANES, LANES), 1)
                - lax.broadcasted_iota(jnp.int32, (SUBLANES, LANES), 0))

        gi = 0
        acc = None
        for c in range(nch):
            in_copy(c).wait()
            if c == n1:
                part_rdma.wait_recv()
            if c < n2:
                for b in range(chunks[c] // LANES):
                    r0 = offs[c] + b * LANES
                    if c < n1:
                        part[:, pl.ds(r0, LANES)] = to_lanes(colmax(xbuf, r0, LANES))
                    elif r0 - half >= raw:
                        q = r0 - half
                        store_final(q, jnp.maximum(to_lanes(colmax(xbuf, r0, LANES)),
                                                   rbuf[:, pl.ds(q, LANES)]))
            else:
                for t in range(chunks[c] // SUBLANES):
                    r0 = offs[c] + t * SUBLANES
                    o = (r0 - half) % LANES
                    q = (r0 - half) - o
                    if o == 0:
                        acc = jnp.broadcast_to(rbuf[:, pl.ds(q, LANES)], (SUBLANES, LANES))
                    r = jnp.max(colmax(xbuf, r0, SUBLANES), axis=1, keepdims=True)
                    acc = jnp.maximum(acc, jnp.where(diag == o, r, -jnp.inf))
                    if o == LANES - SUBLANES:
                        store_final(q, jnp.max(acc, axis=0, keepdims=True))
                        fin_rdma(gi, base2).start()
                        gi += 1
            if c == n1 - 1:
                part_rdma.start()
            if c - n1 == raw_after:
                raw_rdma.wait_recv()
                for b in range(raw // LANES):
                    q = b * LANES
                    store_final(q, to_lanes(jnp.maximum(colmax(xbuf, half + q, LANES),
                                                        colmax(rawbuf, q, LANES))))
            if n1 <= c < n2 and (c - n1) in fin_after:
                fin_rdma(gi, base2).start()
                gi += 1

        part_rdma.wait_send()
        raw_rdma.wait_send()
        for g in range(ng):
            fin_rdma(g, base2).wait_send()
        for g in range(ng):
            fin_rdma(g, base1).wait_recv()

    out = pl.pallas_call(
        body,
        out_shape=jax.ShapeDtypeStruct((1, m), x.dtype),
        in_specs=[pl.BlockSpec(memory_space=pl.ANY)],
        out_specs=pl.BlockSpec(memory_space=pltpu.VMEM),
        scratch_shapes=[
            pltpu.VMEM((m, n), x.dtype),
            pltpu.VMEM((raw, n), x.dtype),
            pltpu.VMEM((1, half), x.dtype),
            pltpu.VMEM((1, half), x.dtype),
            pltpu.SemaphoreType.DMA((nch,)),
            pltpu.SemaphoreType.DMA,
            pltpu.SemaphoreType.DMA,
            pltpu.SemaphoreType.DMA((ng,)),
            pltpu.SemaphoreType.DMA((ng,)),
            pltpu.SemaphoreType.DMA,
            pltpu.SemaphoreType.DMA,
        ],
        compiler_params=pltpu.CompilerParams(
            collective_id=0,
            disable_semaphore_checks=True,
            disable_bounds_checks=True,
            vmem_limit_bytes=64 * 1024 * 1024),
    )(x)
    return out.reshape(m, 1)
```

```python
import jax
import jax.numpy as jnp
from jax import lax
from jax.experimental import pallas as pl
from jax.experimental.pallas import tpu as pltpu

LANES = 128


def pallas_dist_max_ax1_xy_m4096_n1024_kernel(
x: jax.Array,
):
    m, n = x.shape
    half = m // 2
    raw_chunks = (128, 64)
    raw_after = (1, 2)
    raw = sum(raw_chunks)
    raw_full = (raw // LANES) * LANES
    chunks1 = (half // 2 - raw, half // 2)
    chunks2 = (half // 2, half // 4, half // 8, half // 8 - LANES)
    tail = (64, 32, 32)
    fin_after = (2, 3)

    chunks = chunks1 + chunks2 + tail
    n1 = len(chunks1)
    n2 = n1 + len(chunks2)
    nch = len(chunks)
    offs = [raw + sum(chunks[:i]) for i in range(nch)]
    assert offs[n1] == half and offs[-1] + chunks[-1] == m and sum(tail) == LANES
    groups = []
    prev = 0
    for f in fin_after:
        end = sum(chunks2[:f + 1])
        groups.append((prev, end - prev))
        prev = end
    groups.append((prev, LANES))
    ng = len(groups)
    nraw = len(raw_chunks)
    roffs = [sum(raw_chunks[:i]) for i in range(nraw)]

    def body(x_hbm, out_ref, xbuf, rawbuf, pm, rbuf,
             in_sems, p_send, p_recv, f_send, f_recv, r_send, r_recv):
        my_x = lax.axis_index("x")
        my_y = lax.axis_index("y")
        nbr = (my_x, 1 - my_y)
        base1 = pl.multiple_of(my_y * half, half)
        base2 = pl.multiple_of((1 - my_y) * half, half)

        def in_copy(c):
            g = (base1 + offs[c]) if c < n1 else (base2 + (offs[c] - half))
            return pltpu.make_async_copy(
                x_hbm.at[pl.ds(g, chunks[c]), :],
                xbuf.at[pl.ds(offs[c], chunks[c]), :],
                in_sems.at[c])

        for c in range(nch):
            in_copy(c).start()

        barrier = pltpu.get_barrier_semaphore()
        pl.semaphore_signal(barrier, inc=1, device_id=nbr,
                            device_id_type=pl.DeviceIdType.MESH)
        pl.semaphore_wait(barrier, 1)

        def raw_rdma(i):
            return pltpu.make_async_remote_copy(
                src_ref=x_hbm.at[pl.ds(base1 + roffs[i], raw_chunks[i]), :],
                dst_ref=rawbuf.at[pl.ds(roffs[i], raw_chunks[i]), :],
                send_sem=r_send.at[i], recv_sem=r_recv.at[i],
                device_id=nbr, device_id_type=pl.DeviceIdType.MESH)

        for i in range(nraw):
            raw_rdma(i).start()

        part_rdma = pltpu.make_async_remote_copy(
            src_ref=pm.at[:, pl.ds(raw_full, half - raw_full)],
            dst_ref=rbuf.at[:, pl.ds(raw_full, half - raw_full)],
            send_sem=p_send, recv_sem=p_recv,
            device_id=nbr, device_id_type=pl.DeviceIdType.MESH)

        def fin_rdma(g, base):
            s, l = groups[g]
            sl = out_ref.at[:, pl.ds(base + s, l)]
            return pltpu.make_async_remote_copy(
                src_ref=sl, dst_ref=sl,
                send_sem=f_send.at[g], recv_sem=f_recv.at[g],
                device_id=nbr, device_id_type=pl.DeviceIdType.MESH)

        def rows_to_lanes(buf, r0, nr, lane0):
            vs = [buf[pl.ds(r0, nr), pl.ds(j * LANES, LANES)] for j in range(n // LANES)]
            while len(vs) > 1:
                vs = [jnp.maximum(vs[i], vs[i + 1]) for i in range(0, len(vs), 2)]
            r = jnp.max(vs[0], axis=1, keepdims=True)
            d = (lax.broadcasted_iota(jnp.int32, (nr, LANES), 1)
                 - lax.broadcasted_iota(jnp.int32, (nr, LANES), 0))
            return jnp.max(jnp.where(d == lane0, r, -jnp.inf), axis=0, keepdims=True)

        def local_rows(lo, hi):
            if lo % LANES:
                k = lo % LANES
                pm[:, pl.ds(lo - k, LANES)] = rows_to_lanes(xbuf, lo, LANES - k, k)
                lo += LANES - k
            nb = (hi - lo) // LANES
            if nb > 2:
                def step(i, carry):
                    r0 = pl.multiple_of(lo + i * LANES, LANES)
                    pm[:, pl.ds(r0, LANES)] = rows_to_lanes(xbuf, r0, LANES, 0)
                    return carry
                lax.fori_loop(0, nb, step, 0, unroll=2 if nb % 2 == 0 else 1)
            else:
                for b in range(nb):
                    r0 = lo + b * LANES
                    pm[:, pl.ds(r0, LANES)] = rows_to_lanes(xbuf, r0, LANES, 0)

        def store_final(s, l, val):
            out_ref[:, pl.ds(pl.multiple_of(base2 + s, LANES), l)] = val

        gi = 0
        acc = None
        for c in range(nch):
            in_copy(c).wait()
            lo, hi = offs[c], offs[c] + chunks[c]
            if c < n2:
                local_rows(lo, hi)
            else:
                if c == n2:
                    acc = rbuf[:, pl.ds(half - LANES, LANES)]
                acc = jnp.maximum(acc, rows_to_lanes(xbuf, lo, hi - lo, lo % LANES))
                if c == nch - 1:
                    store_final(half - LANES, LANES, acc)
                    fin_rdma(gi, base2).start()
                    gi += 1
            if c == n1 - 1:
                part_rdma.start()
            for i in range(nraw):
                if c - n1 == raw_after[i]:
                    raw_rdma(i).wait_recv()
                    dst = pl.ds(half + roffs[i], LANES)
                    pm[:, dst] = jnp.maximum(
                        pm[:, dst], rows_to_lanes(rawbuf, roffs[i], raw_chunks[i], 0))
            if n1 <= c < n2 and (c - n1) in fin_after:
                s, l = groups[gi]
                if gi == 0:
                    part_rdma.wait_recv()
                    store_final(0, raw_full, pm[:, pl.ds(half, raw_full)])
                    s, l = raw_full, l - raw_full
                store_final(s, l, jnp.maximum(pm[:, pl.ds(half + s, l)],
                                              rbuf[:, pl.ds(s, l)]))
                fin_rdma(gi, base2).start()
                gi += 1

        part_rdma.wait_send()
        for i in range(nraw):
            raw_rdma(i).wait_send()
        for g in range(ng):
            fin_rdma(g, base2).wait_send()
        for g in range(ng):
            fin_rdma(g, base1).wait_recv()

    out = pl.pallas_call(
        body,
        out_shape=jax.ShapeDtypeStruct((1, m), x.dtype),
        in_specs=[pl.BlockSpec(memory_space=pl.ANY)],
        out_specs=pl.BlockSpec(memory_space=pltpu.VMEM),
        scratch_shapes=[
            pltpu.VMEM((m, n), x.dtype),
            pltpu.VMEM((raw, n), x.dtype),
            pltpu.VMEM((1, m), x.dtype),
            pltpu.VMEM((1, half), x.dtype),
            pltpu.SemaphoreType.DMA((nch,)),
            pltpu.SemaphoreType.DMA,
            pltpu.SemaphoreType.DMA,
            pltpu.SemaphoreType.DMA((ng,)),
            pltpu.SemaphoreType.DMA((ng,)),
            pltpu.SemaphoreType.DMA((nraw,)),
            pltpu.SemaphoreType.DMA((nraw,)),
        ],
        compiler_params=pltpu.CompilerParams(
            collective_id=0,
            disable_semaphore_checks=True,
            disable_bounds_checks=True,
            vmem_limit_bytes=64 * 1024 * 1024),
    )(x)
    return out.reshape(m, 1)
```
